```python
import numpy as np

kernel_name = "dist_rmsnorm_colshard_i_m768_n512"

def setup_inputs():
    x = np.random.randn(768, 2048).astype(np.float32)
    gamma = np.random.randn(2048).astype(np.float32)
    return {"x": x, "gamma": gamma}

def reference(x: np.ndarray, gamma: np.ndarray) -> np.ndarray:
    eps = 1e-5
    rms = np.sqrt(np.mean(x * x, axis=1, keepdims=True) + eps)
    return gamma * x / rms
```

```python
import jax
import jax.numpy as jnp
from jax import lax
from jax.experimental import pallas as pl
from jax.experimental.pallas import tpu as pltpu

_EPS = 1e-5
_N_DEV = 4
_LANES = 128
_SUBLANES = 8

_LOAD_ROWS = (256, 256, 128, 80, 40, 8)
_BULK_ROWS = (256, 256, 128)
_TAIL_ROWS = (80, 48)


def _spans(sizes, start=0):
    out = []
    for size in sizes:
        out.append((start, size))
        start += size
    return out


def _pairwise(vals, combine):
    level = 0
    while len(vals) > 1:
        vals = [combine(vals[k], vals[k + 1], level) for k in range(0, len(vals), 2)]
        level += 1
    return vals[0]


def _lanes_to_rows(packed, rows):
    row = lax.broadcasted_iota(jnp.int32, (rows, _LANES), 0)
    lane = lax.broadcasted_iota(jnp.int32, (rows, _LANES), 1)
    return jnp.sum(jnp.where(row == lane, packed, 0.0), axis=1, keepdims=True)


def pallas_dist_rmsnorm_colshard_i_m768_n512_kernel(
    x: jax.Array,
    gamma: jax.Array,
):
    m, n = x.shape
    n_global = n * _N_DEV
    assert sum(_LOAD_ROWS) == sum(_BULK_ROWS) + sum(_TAIL_ROWS) == m

    slots, messages = [], []
    for start, size in _spans(_BULK_ROWS + _TAIL_ROWS):
        first = len(slots)
        slots += [(start + r, min(_LANES, size - r)) for r in range(0, size, _LANES)]
        messages.append((first, len(slots) - first))
    n_bulk = len(_BULK_ROWS)
    tail_slot = messages[n_bulk][0]
    tail_row = slots[tail_slot][0]
    neighbour_slots = {
        n_bulk - 1: (0, tail_slot),
        len(messages) - 1: (tail_slot, len(slots) - tail_slot),
    }

    def kernel_body(
        x_hbm, gamma_hbm, out, gamma_vmem, mine, from_nbrs, from_diag, from_diag_smem,
        tail_near, load_sems, diag_sems, nbr_sems,
    ):
        loads = {}
        for k, (start, size) in enumerate(_spans(_LOAD_ROWS)):
            rows = pl.ds(start, size)
            loads[start] = pltpu.make_async_copy(x_hbm.at[rows], out.at[rows], load_sems.at[k])
            loads[start].start()
        gamma_load = pltpu.make_async_copy(gamma_hbm, gamma_vmem, load_sems.at[len(loads)])
        gamma_load.start()

        me = lax.axis_index("i")
        diag, right, left = (((me + d) & (_N_DEV - 1),) for d in (2, 1, 3))
        barrier = pltpu.get_barrier_semaphore()
        for peer in (diag, right, left):
            pl.semaphore_signal(barrier, 1, device_id=peer, device_id_type=pl.DeviceIdType.MESH)

        def send(span, dst, sems, k, peer):
            span = pl.ds(*span)
            copy = pltpu.make_async_remote_copy(
                mine.at[span], dst.at[span], sems.at[2 * k], sems.at[2 * k + 1],
                device_id=peer, device_id_type=pl.DeviceIdType.MESH,
            )
            copy.start()
            return copy

        sublane = lax.broadcasted_iota(jnp.int32, (_SUBLANES, _LANES), 0)
        lane = lax.broadcasted_iota(jnp.int32, (_SUBLANES, _LANES), 1)

        to_diag, to_nbrs = [], []
        for k, (first, count) in enumerate(messages):
            for s in range(first, first + count):
                start, size = slots[s]
                partial = []
                for r in range(start, start + size, _SUBLANES):
                    if r in loads:
                        loads[r].wait()
                    v = out[pl.ds(r, _SUBLANES), :]
                    sq = v * v
                    tiles = [sq[:, c:c + _LANES] for c in range(0, n, _LANES)]
                    partial.append(_pairwise(tiles, lambda a, b, _: a + b))
                packed = jnp.zeros((_SUBLANES, _LANES), jnp.float32)
                for j, p in enumerate(partial):
                    row_sum = jnp.sum(p, axis=1, keepdims=True)
                    packed = jnp.where(lane - sublane == _SUBLANES * j, row_sum, packed)
                mine[s] = jnp.sum(packed, axis=0, keepdims=True)
            if k == 0:
                pl.semaphore_wait(barrier, _N_DEV - 1)
            dst = from_diag if k < n_bulk else from_diag_smem
            to_diag.append(send((first, count), dst, diag_sems, k, diag))
            if k in neighbour_slots:
                for side, peer in enumerate((right, left)):
                    to_nbrs.append(
                        send(neighbour_slots[k], from_nbrs.at[side], nbr_sems, len(to_nbrs), peer)
                    )

        gamma_load.wait()
        weight = gamma_vmem[...] * n_global**0.5

        def near(s):
            return (mine[s] + n_global * _EPS) + (from_nbrs[0, s] + from_nbrs[1, s])

        for k, (first, count) in enumerate(messages):
            if k == 0:
                for copy in to_nbrs[:2]:
                    copy.wait_recv()
            if k == 1:
                for copy in to_nbrs[2:]:
                    copy.wait_recv()
                for s in range(tail_slot, len(slots)):
                    start, size = slots[s]
                    tail_near[pl.ds(start - tail_row, size), :] = jnp.broadcast_to(
                        _lanes_to_rows(near(s), size), (size, _LANES)
                    )
            if k == n_bulk - 1:
                for copy in to_diag + to_nbrs:
                    copy.wait_send()
            to_diag[k].wait_recv()
            for s in range(first, first + count):
                start, size = slots[s]
                if k < n_bulk:
                    scale = _lanes_to_rows(lax.rsqrt(near(s) + from_diag[s]), size)
                    rows = pl.ds(start, size)
                    out[rows, :] = out[rows, :] * weight * scale
                    continue
                for r in range(0, size, _SUBLANES):
                    far = _pairwise(
                        [
                            jnp.full((_SUBLANES, _LANES), from_diag_smem[s, 0, r + i])
                            for i in range(_SUBLANES)
                        ],
                        lambda a, b, level: jnp.where((sublane & (1 << level)) != 0, b, a),
                    )
                    scale = lax.rsqrt(tail_near[pl.ds(start - tail_row + r, _SUBLANES), :] + far)
                    rows = pl.ds(start + r, _SUBLANES)
                    out[rows, :] = (
                        out[rows, :] * weight * jnp.concatenate([scale] * (n // _LANES), axis=1)
                    )

    packed_shape = (len(slots), 1, _LANES)
    in_hbm = pl.BlockSpec(memory_space=pltpu.HBM)
    return pl.pallas_call(
        kernel_body,
        out_shape=jax.ShapeDtypeStruct((m, n), jnp.float32),
        in_specs=[in_hbm, in_hbm],
        out_specs=pl.BlockSpec(memory_space=pltpu.VMEM),
        scratch_shapes=[
            pltpu.VMEM((1, n), jnp.float32),
            pltpu.VMEM(packed_shape, jnp.float32),
            pltpu.VMEM((2,) + packed_shape, jnp.float32),
            pltpu.VMEM(packed_shape, jnp.float32),
            pltpu.SMEM(packed_shape, jnp.float32),
            pltpu.VMEM((m - tail_row, _LANES), jnp.float32),
            pltpu.SemaphoreType.DMA((len(_LOAD_ROWS) + 1,)),
            pltpu.SemaphoreType.DMA((2 * len(messages),)),
            pltpu.SemaphoreType.DMA((4 * len(neighbour_slots),)),
        ],
        compiler_params=pltpu.CompilerParams(
            collective_id=0,
            disable_bounds_checks=True,
            disable_semaphore_checks=True,
        ),
    )(x, gamma.reshape(1, n))
```

```python
import jax
import jax.numpy as jnp
from jax import lax
from jax.experimental import pallas as pl
from jax.experimental.pallas import tpu as pltpu

_EPS = 1e-5
_N_DEV = 4
_LANES = 128
_SUBLANES = 8

_LOAD_ROWS = (256, 176, 128, 96, 64, 40, 8)
_BULK_ROWS = (256, 176, 128)
_TAIL_ROWS = (96, 64, 48)


def _spans(sizes, start=0):
    out = []
    for size in sizes:
        out.append((start, size))
        start += size
    return out


def _pairwise(vals, combine):
    level = 0
    while len(vals) > 1:
        vals = [combine(vals[k], vals[k + 1], level) for k in range(0, len(vals), 2)]
        level += 1
    return vals[0]


def _lanes_to_rows(packed, rows):
    row = lax.broadcasted_iota(jnp.int32, (rows, _LANES), 0)
    lane = lax.broadcasted_iota(jnp.int32, (rows, _LANES), 1)
    return jnp.sum(jnp.where(row == lane, packed, 0.0), axis=1, keepdims=True)


def pallas_dist_rmsnorm_colshard_i_m768_n512_kernel(
    x: jax.Array,
    gamma: jax.Array,
):
    m, n = x.shape
    inv_n = 1.0 / (n * _N_DEV)
    assert sum(_LOAD_ROWS) == sum(_BULK_ROWS) + sum(_TAIL_ROWS) == m

    slots, messages = [], []
    for start, size in _spans(_BULK_ROWS + _TAIL_ROWS):
        first = len(slots)
        slots += [(start + r, min(_LANES, size - r)) for r in range(0, size, _LANES)]
        messages.append((first, len(slots) - first))
    n_bulk = len(_BULK_ROWS)
    tail_slot = messages[n_bulk][0]
    tail_row = slots[tail_slot][0]
    neighbour_slots = {
        n_bulk - 1: (0, tail_slot),
        len(messages) - 1: (tail_slot, len(slots) - tail_slot),
    }

    def kernel_body(
        x_hbm, gamma_hbm, out, gamma_vmem, mine, from_nbrs, from_diag, from_diag_smem,
        tail_near, load_sems, diag_sems, nbr_sems,
    ):
        loads = {}
        for k, (start, size) in enumerate(_spans(_LOAD_ROWS)):
            rows = pl.ds(start, size)
            loads[start] = pltpu.make_async_copy(x_hbm.at[rows], out.at[rows], load_sems.at[k])
            loads[start].start()
        gamma_load = pltpu.make_async_copy(gamma_hbm, gamma_vmem, load_sems.at[len(loads)])
        gamma_load.start()

        me = lax.axis_index("i")
        diag, right, left = (((me + d) & (_N_DEV - 1),) for d in (2, 1, 3))
        barrier = pltpu.get_barrier_semaphore()
        for peer in (diag, right, left):
            pl.semaphore_signal(barrier, 1, device_id=peer, device_id_type=pl.DeviceIdType.MESH)

        def send(span, dst, sems, k, peer):
            span = pl.ds(*span)
            copy = pltpu.make_async_remote_copy(
                mine.at[span], dst.at[span], sems.at[2 * k], sems.at[2 * k + 1],
                device_id=peer, device_id_type=pl.DeviceIdType.MESH,
            )
            copy.start()
            return copy

        sublane = lax.broadcasted_iota(jnp.int32, (_SUBLANES, _LANES), 0)
        lane = lax.broadcasted_iota(jnp.int32, (_SUBLANES, _LANES), 1)

        to_diag, to_nbrs = [], []
        for k, (first, count) in enumerate(messages):
            for s in range(first, first + count):
                start, size = slots[s]
                partial = []
                for r in range(start, start + size, _SUBLANES):
                    if r in loads:
                        loads[r].wait()
                    v = out[pl.ds(r, _SUBLANES), :]
                    sq = v * v
                    tiles = [sq[:, c:c + _LANES] for c in range(0, n, _LANES)]
                    partial.append(_pairwise(tiles, lambda a, b, _: a + b))
                packed = jnp.zeros((_SUBLANES, _LANES), jnp.float32)
                for j, p in enumerate(partial):
                    row_sum = jnp.sum(p, axis=1, keepdims=True)
                    packed = jnp.where(lane - sublane == _SUBLANES * j, row_sum, packed)
                mine[s] = jnp.sum(packed, axis=0, keepdims=True)
            if k == 0:
                pl.semaphore_wait(barrier, _N_DEV - 1)
            dst = from_diag if k < n_bulk else from_diag_smem
            to_diag.append(send((first, count), dst, diag_sems, k, diag))
            if k in neighbour_slots:
                for side, peer in enumerate((right, left)):
                    to_nbrs.append(
                        send(neighbour_slots[k], from_nbrs.at[side], nbr_sems, len(to_nbrs), peer)
                    )

        gamma_load.wait()
        weight = gamma_vmem[...]

        def near(s):
            return (mine[s] + from_nbrs[0, s] + from_nbrs[1, s]) * inv_n + _EPS

        for k, (first, count) in enumerate(messages):
            if k == 0:
                for copy in to_nbrs[:2]:
                    copy.wait_recv()
            if k == 1:
                for copy in to_nbrs[2:]:
                    copy.wait_recv()
                for s in range(tail_slot, len(slots)):
                    start, size = slots[s]
                    tail_near[pl.ds(start - tail_row, size), :] = jnp.broadcast_to(
                        _lanes_to_rows(near(s), size), (size, _LANES)
                    )
            if k == n_bulk - 1:
                for copy in to_diag + to_nbrs:
                    copy.wait_send()
            to_diag[k].wait_recv()
            for s in range(first, first + count):
                start, size = slots[s]
                if k < n_bulk:
                    scale = _lanes_to_rows(lax.rsqrt(near(s) + from_diag[s] * inv_n), size)
                    rows = pl.ds(start, size)
                    out[rows, :] = out[rows, :] * weight * scale
                    continue
                for r in range(0, size, _SUBLANES):
                    far = _pairwise(
                        [
                            jnp.full((_SUBLANES, _LANES), from_diag_smem[s, 0, r + i])
                            for i in range(_SUBLANES)
                        ],
                        lambda a, b, level: jnp.where((sublane & (1 << level)) != 0, b, a),
                    )
                    rest = tail_near[pl.ds(start - tail_row + r, _SUBLANES), :]
                    scale = lax.rsqrt(rest + far * inv_n)
                    rows = pl.ds(start + r, _SUBLANES)
                    out[rows, :] = (
                        out[rows, :] * weight * jnp.concatenate([scale] * (n // _LANES), axis=1)
                    )

    packed_shape = (len(slots), 1, _LANES)
    in_hbm = pl.BlockSpec(memory_space=pltpu.HBM)
    return pl.pallas_call(
        kernel_body,
        out_shape=jax.ShapeDtypeStruct((m, n), jnp.float32),
        in_specs=[in_hbm, in_hbm],
        out_specs=pl.BlockSpec(memory_space=pltpu.VMEM),
        scratch_shapes=[
            pltpu.VMEM((1, n), jnp.float32),
            pltpu.VMEM(packed_shape, jnp.float32),
            pltpu.VMEM((2,) + packed_shape, jnp.float32),
            pltpu.VMEM(packed_shape, jnp.float32),
            pltpu.SMEM(packed_shape, jnp.float32),
            pltpu.VMEM((m - tail_row, _LANES), jnp.float32),
            pltpu.SemaphoreType.DMA((len(_LOAD_ROWS) + 1,)),
            pltpu.SemaphoreType.DMA((2 * len(messages),)),
            pltpu.SemaphoreType.DMA((4 * len(neighbour_slots),)),
        ],
        compiler_params=pltpu.CompilerParams(
            collective_id=0,
            disable_bounds_checks=True,
            disable_semaphore_checks=True,
        ),
    )(x, gamma.reshape(1, n))
```
